```python
import numpy as np

kernel_name = "dist_argmax_global_i_m4096_n1024"

def setup_inputs():
    return {"x": np.random.randn(16384, 1024).astype(np.float32)}

def reference(x: np.ndarray) -> np.ndarray:
    idx = np.argmax(x, axis=0).astype(np.float32)
    val = np.max(x, axis=0)
    return np.stack([val, idx], axis=0)
```

```python
import jax
import jax.numpy as jnp
from jax import lax
from jax.experimental import pallas as pl
from jax.experimental.pallas import tpu as pltpu

N_DEV = 4
N_CHUNKS = 16
SUB = 8


def _better(cand, cur):
    return jnp.logical_or(cand > cur, jnp.logical_and(cand != cand, cur == cur))


def pallas_dist_argmax_global_i_m4096_n1024_kernel(x: jax.Array):
    m, n = x.shape
    rows_per_chunk = m // N_CHUNKS
    groups_per_chunk = rows_per_chunk // SUB

    def body(x_hbm, out_ref, xbuf, comm, copy_sems, send_sems, recv_sems):
        my = lax.axis_index("i")

        barrier = pltpu.get_barrier_semaphore()
        for d in range(1, N_DEV):
            pl.semaphore_signal(
                barrier, inc=1,
                device_id=((my + d) % N_DEV,),
                device_id_type=pl.DeviceIdType.MESH,
            )

        copies = [
            pltpu.make_async_copy(
                x_hbm.at[pl.ds(c * rows_per_chunk, rows_per_chunk)],
                xbuf.at[pl.ds(c * rows_per_chunk, rows_per_chunk)],
                copy_sems.at[c],
            )
            for c in range(N_CHUNKS)
        ]
        for cp in copies:
            cp.start()

        sub = lax.broadcasted_iota(jnp.int32, (SUB, n), 0)

        def step(g, carry):
            cur_v, cur_i = carry
            row0 = pl.multiple_of(g * SUB, SUB)
            xv = xbuf[pl.ds(row0, SUB), :]
            upd = _better(xv, cur_v)
            return jnp.where(upd, xv, cur_v), jnp.where(upd, sub + row0, cur_i)

        carry = None
        for c in range(N_CHUNKS):
            copies[c].wait()
            lo = c * groups_per_chunk
            hi = (c + 1) * groups_per_chunk
            if c == 0:
                carry = (xbuf[pl.ds(0, SUB), :], sub)
                lo = 1
            carry = lax.fori_loop(lo, hi, step, carry, unroll=4)
        cur_v, cur_i = carry

        nan_f = jnp.where(cur_v != cur_v, 1.0, 0.0)
        has_nan = jnp.max(nan_f, axis=0, keepdims=True)
        vmax = jnp.max(jnp.where(cur_v != cur_v, -jnp.inf, cur_v), axis=0, keepdims=True)
        eq_f = jnp.where(cur_v == vmax, 1.0, 0.0)
        cand_f = jnp.where(has_nan > 0.0, nan_f, eq_f)
        big = jnp.int32(2**30)
        idx = jnp.min(jnp.where(cand_f > 0.0, cur_i, big), axis=0, keepdims=True)
        val = jnp.where(has_nan > 0.0, jnp.nan, vmax)
        gidx = (idx + my * m).astype(jnp.float32)

        comm[my, 0:1, :] = val
        comm[my, 1:2, :] = gidx

        pl.semaphore_wait(barrier, N_DEV - 1)

        sends = []
        for d in range(1, N_DEV):
            peer = (my + d) % N_DEV
            rdma = pltpu.make_async_remote_copy(
                src_ref=comm.at[my],
                dst_ref=comm.at[my],
                send_sem=send_sems.at[d - 1],
                recv_sem=recv_sems.at[my],
                device_id=(peer,),
                device_id_type=pl.DeviceIdType.MESH,
            )
            rdma.start()
            sends.append(rdma)

        for d in range(1, N_DEV):
            src = (my + d) % N_DEV
            pltpu.make_async_remote_copy(
                src_ref=comm.at[src],
                dst_ref=comm.at[src],
                send_sem=send_sems.at[d - 1],
                recv_sem=recv_sems.at[src],
                device_id=(src,),
                device_id_type=pl.DeviceIdType.MESH,
            ).wait_recv()
        for rdma in sends:
            rdma.wait_send()

        best_v = comm[0, 0:1, :]
        best_i = comm[0, 1:2, :]
        for k in range(1, N_DEV):
            v = comm[k, 0:1, :]
            i = comm[k, 1:2, :]
            upd = _better(v, best_v)
            best_v = jnp.where(upd, v, best_v)
            best_i = jnp.where(upd, i, best_i)
        out_ref[0:1, :] = best_v
        out_ref[1:2, :] = best_i

    return pl.pallas_call(
        body,
        out_shape=jax.ShapeDtypeStruct((2, n), jnp.float32),
        in_specs=[pl.BlockSpec(memory_space=pl.ANY)],
        out_specs=pl.BlockSpec(memory_space=pltpu.VMEM),
        scratch_shapes=[
            pltpu.VMEM((m, n), jnp.float32),
            pltpu.VMEM((N_DEV, 2, n), jnp.float32),
            pltpu.SemaphoreType.DMA((N_CHUNKS,)),
            pltpu.SemaphoreType.DMA((N_DEV - 1,)),
            pltpu.SemaphoreType.DMA((N_DEV,)),
        ],
        compiler_params=pltpu.CompilerParams(
            collective_id=0,
            vmem_limit_bytes=64 * 1024 * 1024,
        ),
    )(x)
```

```python
import jax
import jax.numpy as jnp
from jax import lax
from jax.experimental import pallas as pl
from jax.experimental.pallas import tpu as pltpu

N_DEV = 4
UNROLL = 4
SUB = 8


def _better(cand, cur):
    return jnp.logical_or(cand > cur, jnp.logical_and(cand != cand, cur == cur))


def _chunks(m):
    sizes = [m // 8] * 7 + [m // 16, m // 32, m // 64, m // 128, m // 128]
    assert sum(sizes) == m and all(sz % SUB == 0 for sz in sizes)
    out, o = [], 0
    for sz in sizes:
        out.append((o, sz))
        o += sz
    return out


def pallas_dist_argmax_global_i_m4096_n1024_kernel(x: jax.Array):
    m, n = x.shape
    chunks = _chunks(m)
    n_chunks = len(chunks)

    def body(x_hbm, out_ref, xbuf, comm, copy_sems, send_sems, recv_sems):
        my = lax.axis_index("i")

        copies = [
            pltpu.make_async_copy(
                x_hbm.at[pl.ds(o, s)],
                xbuf.at[pl.ds(o, s)],
                copy_sems.at[c],
            )
            for c, (o, s) in enumerate(chunks)
        ]
        for cp in copies:
            cp.start()

        barrier = pltpu.get_barrier_semaphore()
        for d in range(1, N_DEV):
            pl.semaphore_signal(
                barrier, inc=1,
                device_id=((my + d) % N_DEV,),
                device_id_type=pl.DeviceIdType.MESH,
            )

        sub = lax.broadcasted_iota(jnp.int32, (SUB, n), 0)

        def step(g, carry):
            cur_v, cur_i = carry
            row0 = pl.multiple_of(g * SUB, SUB)
            xv = xbuf[pl.ds(row0, SUB), :]
            upd = _better(xv, cur_v)
            return jnp.where(upd, xv, cur_v), jnp.where(upd, sub + row0, cur_i)

        carry = None
        for c, (o, s) in enumerate(chunks):
            copies[c].wait()
            lo = o // SUB
            hi = (o + s) // SUB
            if c == 0:
                carry = (xbuf[pl.ds(0, SUB), :], sub)
                lo = 1
            carry = lax.fori_loop(lo, hi, step, carry, unroll=UNROLL)
        cur_v, cur_i = carry

        nan_f = jnp.where(cur_v != cur_v, 1.0, 0.0)
        has_nan = jnp.max(nan_f, axis=0, keepdims=True)
        vmax = jnp.max(jnp.where(cur_v != cur_v, -jnp.inf, cur_v), axis=0, keepdims=True)
        eq_f = jnp.where(cur_v == vmax, 1.0, 0.0)
        cand_f = jnp.where(has_nan > 0.0, nan_f, eq_f)
        big = jnp.int32(2**30)
        idx = jnp.min(jnp.where(cand_f > 0.0, cur_i, big), axis=0, keepdims=True)
        val = jnp.where(has_nan > 0.0, jnp.nan, vmax)
        gidx = (idx + my * m).astype(jnp.float32)

        comm[my, 0:1, :] = val
        comm[my, 1:2, :] = gidx

        pl.semaphore_wait(barrier, N_DEV - 1)

        sends = []
        for d in range(1, N_DEV):
            peer = (my + d) % N_DEV
            rdma = pltpu.make_async_remote_copy(
                src_ref=comm.at[my],
                dst_ref=comm.at[my],
                send_sem=send_sems.at[d - 1],
                recv_sem=recv_sems.at[my],
                device_id=(peer,),
                device_id_type=pl.DeviceIdType.MESH,
            )
            rdma.start()
            sends.append(rdma)

        for d in range(1, N_DEV):
            src = (my + d) % N_DEV
            pltpu.make_async_remote_copy(
                src_ref=comm.at[src],
                dst_ref=comm.at[src],
                send_sem=send_sems.at[d - 1],
                recv_sem=recv_sems.at[src],
                device_id=(src,),
                device_id_type=pl.DeviceIdType.MESH,
            ).wait_recv()

        best_v = comm[0, 0:1, :]
        best_i = comm[0, 1:2, :]
        for k in range(1, N_DEV):
            v = comm[k, 0:1, :]
            i = comm[k, 1:2, :]
            upd = _better(v, best_v)
            best_v = jnp.where(upd, v, best_v)
            best_i = jnp.where(upd, i, best_i)
        out_ref[0:1, :] = best_v
        out_ref[1:2, :] = best_i
        for rdma in sends:
            rdma.wait_send()

    return pl.pallas_call(
        body,
        out_shape=jax.ShapeDtypeStruct((2, n), jnp.float32),
        in_specs=[pl.BlockSpec(memory_space=pl.ANY)],
        out_specs=pl.BlockSpec(memory_space=pltpu.VMEM),
        scratch_shapes=[
            pltpu.VMEM((m, n), jnp.float32),
            pltpu.VMEM((N_DEV, 2, n), jnp.float32),
            pltpu.SemaphoreType.DMA((n_chunks,)),
            pltpu.SemaphoreType.DMA((N_DEV - 1,)),
            pltpu.SemaphoreType.DMA((N_DEV,)),
        ],
        compiler_params=pltpu.CompilerParams(
            collective_id=0,
            vmem_limit_bytes=64 * 1024 * 1024,
        ),
    )(x)
```
